```python
import numpy as np

kernel_name = "dist_sparse_attn_strided_qseq_b1_sq1024_skv1024_hq8_dh128"

def setup_inputs():
    x = np.random.randn(1, 4096, 1024).astype(np.float32)
    Wq = np.random.randn(1024, 4096).astype(np.float32) * 0.02
    K_ext = np.random.randn(1, 1024, 32, 128).astype(np.float32)
    V_ext = np.random.randn(1, 1024, 32, 128).astype(np.float32)
    Wo = np.random.randn(4096, 1024).astype(np.float32) * 0.02
    return {"x": x, "Wq": Wq, "K_ext": K_ext, "V_ext": V_ext, "Wo": Wo}

def reference(x, Wq, K_ext, V_ext, Wo):
    B, Sq, Skv, Hq, Dh = 1, 4096, 1024, 32, 128
    Q = (x @ Wq).reshape(B, Sq, Hq, Dh)
    qb = (np.arange(Sq) // 64)[:, None]
    kb = (np.arange(Skv) // 64)[None, :]
    mask = (qb == kb) | ((kb % 4) == (qb % 4))
    scores = np.einsum('bihd,bjhd->bhij', Q, K_ext).astype(np.float32) * 0.08838834764831843
    scores = np.where(mask[None, None, :, :], scores, -1e9)
    scores_max = scores.max(axis=-1, keepdims=True)
    w = np.exp(scores - scores_max)
    row_keep = mask.any(axis=1)
    w_sum = np.where(row_keep[None, None, :, None], w.sum(axis=-1, keepdims=True), 1.0)
    w = w / w_sum
    w = np.where(row_keep[None, None, :, None], w, 0.0)
    ctx = np.einsum('bhij,bjhd->bihd', w, V_ext).reshape(B, Sq, Hq * Dh)
    return ctx @ Wo
```

```python
from functools import partial
import jax
import jax.numpy as jnp
from jax import lax
from jax.experimental import pallas as pl
from jax.experimental.pallas import tpu as pltpu

F32, BF16, U32 = jnp.float32, jnp.bfloat16, jnp.uint32
SCALE = 0.08838834764831843 * 1.4426950408889634
OWN, NBR = 0, 1


def _schedule():
    ops = []
    a = ops.append
    Q = lambda s, c, g, p: ("Q", s, c, g, p)
    O1 = lambda c, j: ("O", c, OWN, j)
    O2 = lambda c, j: ("O", c, NBR, j)
    PO = lambda c, j: ("PO", c, j)
    pairs = lambda s, c, g, ps=range(4): [(s, c, g, p) for p in ps]

    def attn(units, fill):
        for n, u in enumerate(units):
            a(("S",) + u)
            for f in fill[n:n + 1] if n + 1 < len(units) else fill[n:]:
                ops.extend(f if isinstance(f, list) else [f])
            a(("P",) + u)

    def chain(units, *fill):
        a(("S",) + units[0])
        for u, v in zip(units, units[1:]):
            a(("S",) + v); a(("P",) + u)
        ops.extend(fill); a(("P",) + units[-1])

    def arrive(*what):
        ops.extend(sorted(what, key=lambda op: op[0] not in ("load", "send")))

    kv = lambda g, c: ("loaded", "kv", g, c)
    wo = lambda j: ("loaded", "wo", j)
    send = lambda *arg: ("send",) + arg
    recv = lambda *arg: ("recv",) + arg
    load = lambda *arg: ("load",) + arg

    for i in range(4):
        a(("load", "wq", i)); a(("load", "x", i))
    a(("flush",))
    a(("loaded", "wq", 0)); a(("flush",)); a(("loaded", "x", 0)); a(Q(OWN, 0, OWN, 0))
    arrive(("loaded", "wq", 1)); a(Q(OWN, 0, OWN, 1))
    arrive(("loaded", "x", 1)); a(Q(OWN, 1, OWN, 0)); a(Q(OWN, 1, OWN, 1))
    arrive(("loaded", "wq", 2), load("kv", OWN, 0)); a(Q(OWN, 0, OWN, 2)); a(Q(OWN, 1, OWN, 2))
    arrive(("loaded", "x", 2)); a(Q(OWN, 2, OWN, 0)); a(Q(OWN, 2, OWN, 1))
    arrive(("loaded", "wq", 3), load("kv", OWN, 1)); a(Q(OWN, 2, OWN, 2)); a(Q(OWN, 0, OWN, 3)); a(Q(OWN, 1, OWN, 3))
    arrive(("loaded", "x", 3), load("kv", OWN, 2)); a(Q(OWN, 2, OWN, 3))
    ops.extend(Q(OWN, 3, OWN, p) for p in range(3))
    arrive(recv("wq", 0), load("kv", OWN, 3))
    a(Q(OWN, 3, OWN, 3)); a(Q(OWN, 0, NBR, 0))
    arrive(kv(OWN, 0), recv("x", 0))
    a(Q(OWN, 1, NBR, 0))
    chain(pairs(OWN, 0, OWN, (0, 1)), Q(NBR, 0, OWN, 0))
    chain(pairs(OWN, 0, OWN, (2, 3)), Q(NBR, 0, OWN, 1))
    chain(pairs(NBR, 0, OWN, (0, 1)), load("kv", NBR, 0), kv(OWN, 1), Q(NBR, 0, OWN, 2))
    chain(pairs(OWN, 1, OWN, (0, 1)), Q(NBR, 0, OWN, 3))
    chain(pairs(OWN, 1, OWN, (2, 3)), Q(OWN, 2, NBR, 0))
    chain(pairs(NBR, 0, OWN, (2, 3)), load("kv", NBR, 1), kv(OWN, 2), Q(OWN, 3, NBR, 0))
    chain(pairs(OWN, 2, OWN, (0, 1)), Q(NBR, 0, NBR, 0))
    arrive(recv("wq", 1), load("wo", 0), load("kv", NBR, 2)); a(("flush", 0))
    chain(pairs(OWN, 2, OWN, (2, 3)), Q(OWN, 0, NBR, 1))
    arrive(kv(OWN, 3), recv("x", 1))
    a(Q(OWN, 1, NBR, 1))
    chain(pairs(OWN, 3, OWN, (0, 1)), Q(OWN, 2, NBR, 1))
    chain(pairs(OWN, 3, OWN, (2, 3)), Q(OWN, 3, NBR, 1))
    a(Q(NBR, 1, OWN, 0))
    attn(pairs(NBR, 1, OWN, (0, 1, 2)), [Q(NBR, 1, OWN, 1), Q(NBR, 1, OWN, 2), Q(NBR, 1, OWN, 3)])
    arrive(kv(NBR, 0), kv(NBR, 1), load("wo", 1), load("kv", NBR, 3))
    a(Q(NBR, 0, NBR, 1))
    attn([(NBR, 1, OWN, 3), (NBR, 0, NBR, 0)], [Q(NBR, 1, NBR, 0), Q(NBR, 1, NBR, 1)])
    arrive(recv("wq", 2), load("wo", 2), load("wo", 3)); a(("flush", 0))
    chain([(NBR, 0, NBR, 1)] + pairs(NBR, 1, NBR, (0, 1)), Q(NBR, 0, NBR, 2))
    arrive(recv("x", 2), wo(0))
    a(Q(NBR, 1, NBR, 2)); a(Q(NBR, 2, OWN, 0))
    attn(pairs(NBR, 2, OWN), [Q(NBR, 2, OWN, 1), Q(NBR, 2, OWN, 2), Q(NBR, 2, OWN, 3), O1(0, 0)])
    arrive(kv(NBR, 2), wo(1), send("wo", 0))
    a(Q(NBR, 2, NBR, 0))
    chain([(NBR, 0, NBR, 2), (NBR, 1, NBR, 2)], Q(NBR, 2, NBR, 1))
    chain(pairs(NBR, 2, NBR, (0, 1)), Q(NBR, 2, NBR, 2))
    attn(pairs(NBR, 2, NBR, (2,)), [O1(0, 1)])
    arrive(recv("wq", 3), kv(NBR, 3))
    a(O1(1, 0)); a(Q(NBR, 0, NBR, 3))
    attn([(NBR, 0, NBR, 3)], [Q(NBR, 1, NBR, 3)])
    arrive(recv("x", 3), wo(2), wo(3), send("wo", 1))
    a(Q(NBR, 2, NBR, 3))
    chain([(NBR, 1, NBR, 3), (NBR, 2, NBR, 3)], Q(NBR, 3, OWN, 0))
    attn(pairs(NBR, 3, OWN), [Q(NBR, 3, OWN, 1), Q(NBR, 3, OWN, 2), Q(NBR, 3, OWN, 3), Q(NBR, 3, NBR, 0)])
    attn(pairs(NBR, 3, NBR, (0, 1)), [Q(NBR, 3, NBR, 1), Q(NBR, 3, NBR, 2)])
    arrive(recv("wo", 0))
    a(Q(NBR, 3, NBR, 3)); a(PO(0, 0)); a(send("wo", 2)); a(PO(1, 0))
    attn(pairs(NBR, 3, NBR, (2, 3)), [[send("wo", 3), PO(2, 0)], Q(OWN, 0, NBR, 2)])
    a(PO(3, 0))
    chain(pairs(OWN, 0, NBR, (0, 1)), Q(OWN, 0, NBR, 3))
    chain(pairs(OWN, 0, NBR, (2, 3)), Q(OWN, 1, NBR, 2))
    arrive(recv("wo", 1))
    a(Q(OWN, 1, NBR, 3)); a(PO(0, 1)); a(Q(OWN, 2, NBR, 2))
    attn(pairs(OWN, 1, NBR), [PO(1, 1), PO(2, 1), PO(3, 1), Q(OWN, 2, NBR, 3)])
    chain(pairs(OWN, 2, NBR, (0, 1)), Q(OWN, 3, NBR, 2))
    attn(pairs(OWN, 2, NBR, (2, 3)), [Q(OWN, 3, NBR, 3), O1(2, 0)])
    arrive(recv("wo", 2), *(recv("p", c, 0) for c in range(3)))
    a(O1(1, 1)); a(PO(0, 2)); a(O1(2, 1))
    attn(pairs(OWN, 3, NBR), [PO(1, 2), PO(2, 2), PO(3, 2), O1(0, 2)])
    ops.extend(O1(c, j) for c, j in ((3, 0), (3, 1), (1, 2), (2, 2), (3, 2), (0, 3)))
    arrive(recv("wo", 3), recv("p", 3, 0), *(recv("p", c, 1) for c in range(3)))
    ops.extend(PO(c, 3) for c in range(3))
    arrive(recv("p", 3, 1), *(recv("p", c, 2) for c in range(4)))
    a(PO(3, 3))
    ops.extend(O1(c, 3) for c in range(1, 4))
    for j in range(3):
        for c in range(4):
            a(O2(c, j)); a(("finish", c, j))
    ops.extend(O2(c, 3) for c in range(3))
    arrive(*(recv("p", c, 3) for c in range(3)))
    ops.extend(("finish", c, 3) for c in range(3))
    a(O2(3, 3))
    arrive(recv("p", 3, 3)); a(("finish", 3, 3))
    return ops


def _lhs_terms(a11, a12, a21, a22):
    return a11 + a22, a21 + a22, a11, a22, a11 + a12, a21 - a11, a12 - a22


def _rhs_terms(b11, b12, b21, b22):
    return b11 + b22, b11, b12 - b22, b21 - b11, b22, b11 + b12, b21 + b22


def _pack2(lo, hi):
    return pltpu.bitcast(pltpu.pack_elementwise([lo, hi], packed_dtype=BF16), U32)


def _half(u, i):
    return pltpu.unpack_elementwise(u, index=i, packed_dtype=BF16, unpacked_dtype=F32)


def _pack(v):
    n, w = v.shape
    v = v.reshape(n // 16, 2, 8, w)
    return _pack2(v[:, 0].reshape(n // 2, w), v[:, 1].reshape(n // 2, w))


def _unpack(u):
    return pltpu.bitcast(u, BF16)


def _body(x_hbm, wq_hbm, k_hbm, v_hbm, wo_hbm, out_ref,
          xf, wqf, wof, kf, vf, xb, wqb, wob, ptx, prx, xs, wqs, wos, cs, qb, acc,
          ld_sem, kv_sem, tx_sem, rx_sem):
    me = lax.axis_index("i")
    seq_peer = me ^ 1
    head_peer = 3 - me
    head_shard = (me, head_peer)
    ds = pl.ds

    def remote(src, dst, sem, peer):
        return pltpu.make_async_remote_copy(
            src_ref=src, dst_ref=dst, send_sem=tx_sem.at[sem], recv_sem=rx_sem.at[sem],
            device_id=(peer,), device_id_type=pl.DeviceIdType.MESH)

    cols = lambda j: ds(j * 256, 256)
    load = {
        "x": lambda c: [pltpu.make_async_copy(x_hbm.at[:, c], xf[c], ld_sem.at[c])],
        "wq": lambda p: [pltpu.make_async_copy(wq_hbm.at[:, cols(p)], wqf[p], ld_sem.at[4 + p])],
        "wo": lambda j: [pltpu.make_async_copy(wo_hbm.at[:, cols(j)], wof[j], ld_sem.at[8 + j])],
        "kv": lambda g, c: [
            pltpu.make_async_copy(src.at[:, c, :, head_shard[g]], dst[g][c], kv_sem.at[(g * 4 + c) * 2 + n])
            for n, (src, dst) in enumerate(((k_hbm, kf), (v_hbm, vf)))],
    }
    swap = {
        "x": lambda c: remote(xb[OWN][c], xb[NBR][c], c, seq_peer),
        "wq": lambda p: remote(wqb[OWN][p], wqb[NBR][p], 4 + p, head_peer),
        "wo": lambda j: remote(wob[OWN][j], wob[NBR][j], 8 + j, head_peer),
        "p": lambda c, j: remote(ptx[c][j], prx[c][j], 12 + c * 4 + j, seq_peer),
    }

    first, queue = [], []
    urgent = lambda tag, *fns: first.extend((tag, fn) for fn in fns)
    later = lambda tag, *fns: queue.extend((tag, fn) for fn in fns)

    def drip(n, copies=True):
        if first and not copies:
            return
        while first:
            first.pop(0)[1]()
        for _ in range(min(n, len(queue))):
            queue.pop(0)[1]()

    def need(*tags):
        if any(tag in tags for tag, _ in first):
            drip(0)
        for item in [item for item in queue if item[0] in tags]:
            queue.remove(item)
            item[1]()

    def strassen(lhs, rhs, emit, rate, after_scores):
        def m(i):
            r = jnp.dot(_unpack(lhs(i)), _unpack(rhs(i)), preferred_element_type=F32)
            drip(rate, copies=not after_scores or i in (5, 4, 2))
            return r
        m1, m3 = m(1), m(3)
        emit(1, 0, m1 + m3)
        m0 = m(0)
        c11, c22 = m0 + m3, m0 - m1
        c11 = c11 + m(6)
        c22 = c22 + m(5)
        m4 = m(4)
        emit(0, 0, c11 - m4)
        m2 = m(2)
        emit(1, 1, c22 + m2)
        emit(0, 1, m2 + m4)

    x_slot, wq_slot = {0: 0, 1: 1, 4: 2, 5: 3, 6: 4}, {0: 0, 2: 1, 3: 2, 5: 3, 6: 4}

    def packed_terms(fn, half):
        lo, hi = (fn(*(half(e, i, k) for i in range(2) for k in range(2))) for e in range(2))
        return lambda i: _pack2(lo[i], hi[i])

    def x_terms(s, c, n):
        if s == OWN:
            half = lambda e, i, k: xf[c][2 * i + n // 4, ds(n % 4 * 16 + e * 8, 8), ds(k * 512, 512)]
        else:
            half = lambda e, i, k: _half(xb[s][c][ds(i * 64 + n * 8, 8), ds(k * 512, 512)], e)
        t = packed_terms(_lhs_terms, half)
        for i, slot in x_slot.items():
            xs[s, c, slot, ds(n * 8, 8), :] = t(i)

    def wq_terms(g, p, n):
        half = lambda e, k, i: _half(wqb[g][p][ds(k * 256 + n * 32, 32), ds(i * 128, 128)], e)
        t = packed_terms(_rhs_terms, half)
        for i, slot in wq_slot.items():
            wqs[g, p, slot, ds(n * 32, 32), :] = t(i)

    def wo_terms(g, j, n):
        row = lambda k: n // 2 * 256 + k * 128 + n % 2 * 64
        half = lambda e, k, i: _half(wob[g][j][ds(row(k) // 2, 32), ds(i * 128, 128)], e)
        t = packed_terms(_rhs_terms, half)
        for i in range(7):
            wos[j, i, ds(g * 256 + n * 32, 32), :] = t(i)

    def x_cast(c, n):
        xb[OWN][c][ds(n * 32, 32), :] = _pack(xf[c][n])

    def wq_cast(p, n):
        v = wqf[p][ds(n * 256, 256), :] * SCALE
        wqb[OWN][p][ds(n * 128, 128), :] = pltpu.bitcast(v.astype(BF16), U32)

    def wo_cast(j, n):
        wob[OWN][j][ds(n * 128, 128), :] = pltpu.bitcast(wof[j][ds(n * 256, 256), :].astype(BF16), U32)

    terms = {"x": x_terms, "wq": wq_terms, "wo": wo_terms}
    cast = {"x": x_cast, "wq": wq_cast, "wo": wo_cast}

    def x_term(s, c, i):
        if i in x_slot:
            return xs[s, c, x_slot[i]]
        return xb[s][c][ds(0, 64), ds(0, 512)] if i == 2 else xb[s][c][ds(64, 64), ds(512, 512)]

    def wq_term(g, p, i):
        if i in wq_slot:
            return wqs[g, p, wq_slot[i]]
        return wqb[g][p][ds(0, 256), ds(0, 128)] if i == 1 else wqb[g][p][ds(256, 256), ds(128, 128)]

    def head(ref, g, c, h):
        return ref[g][c].reshape(2048, 128)[ds(h, 256, stride=8), :].astype(BF16)

    def finish(c, j, m):
        mine = acc[c, j, ds(m * 64, 64), :].reshape(4, 2, 8, 256)
        theirs = prx[c][j][ds(m * 32, 32), :]
        r = _pack2(*(mine[:, e].reshape(32, 256) + _half(theirs, e) for e in range(2)))
        out_ref[0, ds((4 * m + c) * 64, 64), cols(j)] = _unpack(r)

    barrier = pltpu.get_barrier_semaphore()
    for peer in (seq_peer, head_peer):
        pl.semaphore_signal(barrier, inc=1, device_id=(peer,), device_id_type=pl.DeviceIdType.MESH)

    probs, sent, issued = {}, [], [None]

    def send(name, *idx):
        swap[name](*idx).start()
        sent.append((name, *idx))

    def run(op, *arg):
        if op == "load":
            urgent(None, lambda: [d.start() for d in load[arg[0]](*arg[1:])])
        elif op == "loaded":
            name, *idx = arg
            tag = (name, *idx) if name == "kv" else (name, OWN, *idx)
            urgent(tag, lambda: [d.wait() for d in load[name](*idx)])
            if name != "kv":
                later(tag, *(partial(cast[name], *idx, k) for k in range(4)))
                if (name, *idx) == ("wq", 0):
                    later(tag, partial(pl.semaphore_wait, barrier, 2))
                if name != "wo":
                    later(tag, partial(send, name, *idx))
                later(tag, *(partial(terms[name], OWN, *idx, k) for k in range(8)))
        elif op == "send":
            name, *idx = arg
            need((name, OWN, *idx))
            urgent(None, partial(send, name, *idx))
        elif op == "recv":
            name, *idx = arg
            tag = (name, NBR, *idx)
            urgent(tag, lambda: swap[name](*idx).wait_recv())
            if name != "p":
                later(tag, *(partial(terms[name], NBR, *idx, k) for k in range(8)))
        elif op == "flush":
            drip(*(arg or [len(queue)]))
        elif op == "Q":
            s, c, g, p = arg
            need(("x", s, c), ("wq", g, p))

            def emit(i, k, v):
                qb[s, c, g, ds(i * 64, 64), ds(p * 256 + k * 128, 128)] = _pack(v)
            strassen(lambda i: x_term(s, c, i), lambda i: wq_term(g, p, i), emit, 1, issued[-1] == "S")
        elif op == "S":
            s, c, g, p = arg
            need(("kv", g, c))
            for h in (2 * p, 2 * p + 1):
                q = _unpack(qb[s, c, g, :, ds(h * 128, 128)])
                sc = lax.dot_general(q, head(kf, g, c, h), (((1,), (1,)), ((), ())), preferred_element_type=F32)
                e = jnp.exp2(sc - jnp.max(sc, axis=1, keepdims=True))
                total = jnp.sum(e, axis=1, keepdims=True)
                r = pl.reciprocal(total, approx=True)
                probs[s, c, g, h] = (e.astype(BF16), r * (2.0 - total * r))
        elif op == "P":
            s, c, g, p = arg
            o = []
            for h in (2 * p, 2 * p + 1):
                e, r = probs.pop((s, c, g, h))
                o.append(jnp.dot(e, head(vf, g, c, h), preferred_element_type=F32) * r)
            for i, t in enumerate(_lhs_terms(o[0][:128], o[1][:128], o[0][128:], o[1][128:])):
                cs[s, c, i, :, ds(g * 512 + p * 128, 128)] = _pack(t)
        elif op == "O":
            c, g, j = arg
            need(("wo", g, j))

            def emit(i, k, v):
                at = (c, j, ds(i * 128, 128), ds(k * 128, 128))
                acc[at] = v if g == OWN else acc[at] + v
            strassen(lambda i: cs[OWN, c, i, :, ds(g * 512, 512)], lambda i: wos[j, i, ds(g * 256, 256), :], emit, 1, issued[-1] == "S")
        elif op == "PO":
            c, j = arg
            need(("wo", OWN, j), ("wo", NBR, j))

            def emit(i, k, v):
                ptx[c][j][ds(i * 64, 64), ds(k * 128, 128)] = _pack(v)
            strassen(lambda i: cs[NBR, c, i], lambda i: wos[j, i], emit, 2, issued[-1] == "S")
            urgent(None, partial(send, "p", c, j))
        elif op == "finish":
            later(None, *(partial(finish, *arg, m) for m in range(4)))
        else:
            raise ValueError(op)
        if op in ("Q", "S", "P", "O", "PO"):
            issued.append(op)

    for step in _schedule():
        run(*step)
    drip(len(queue))
    for name, *idx in sent:
        swap[name](*idx).wait_send()


def pallas_dist_sparse_attn_strided_qseq_b1_sq1024_skv1024_hq8_dh128_kernel(x, Wq, K_ext, V_ext, Wo):
    def bufs(count, shape, dtype):
        if not count:
            return pltpu.VMEM(shape, dtype)
        return [bufs(count[1:], shape, dtype) for _ in range(count[0])]

    hbm = pl.BlockSpec(memory_space=pltpu.MemorySpace.HBM)
    return pl.pallas_call(
        _body,
        out_shape=jax.ShapeDtypeStruct((1, 1024, 1024), BF16),
        in_specs=[hbm] * 5,
        out_specs=pl.BlockSpec(memory_space=pltpu.MemorySpace.VMEM),
        scratch_shapes=[
            bufs((4,), (4, 64, 1024), F32),
            bufs((4,), (1024, 256), F32),
            bufs((4,), (1024, 256), F32),
            bufs((2, 4), (4, 64, 8, 128), F32),
            bufs((2, 4), (4, 64, 8, 128), F32),
            bufs((2, 4), (128, 1024), U32),
            bufs((2, 4), (512, 256), U32),
            bufs((2, 4), (512, 256), U32),
            bufs((4, 4), (128, 256), U32),
            bufs((4, 4), (128, 256), U32),
            pltpu.VMEM((2, 4, 5, 64, 512), U32),
            pltpu.VMEM((2, 4, 5, 256, 128), U32),
            pltpu.VMEM((4, 7, 512, 128), U32),
            pltpu.VMEM((2, 4, 7, 64, 1024), U32),
            pltpu.VMEM((2, 4, 2, 128, 1024), U32),
            pltpu.VMEM((4, 4, 256, 256), F32),
            pltpu.SemaphoreType.DMA((12,)),
            pltpu.SemaphoreType.DMA((16,)),
            pltpu.SemaphoreType.DMA((28,)),
            pltpu.SemaphoreType.DMA((28,)),
        ],
        compiler_params=pltpu.CompilerParams(collective_id=0, vmem_limit_bytes=110 * 1024 * 1024),
    )(x.reshape(4, 4, 64, 1024), Wq, K_ext.reshape(4, 4, 64, 4, 8, 128), V_ext.reshape(4, 4, 64, 4, 8, 128), Wo)
```

```python
from functools import partial
import jax
import jax.numpy as jnp
from jax import lax
from jax.experimental import pallas as pl
from jax.experimental.pallas import tpu as pltpu

F32, BF16, U32 = jnp.float32, jnp.bfloat16, jnp.uint32
SCALE = 0.08838834764831843 * 1.4426950408889634
OWN, NBR = 0, 1


def _schedule():
    ops = []
    a = ops.append
    Q = lambda s, c, g, p: ("Q", s, c, g, p)
    O1 = lambda c, j: ("O", c, OWN, j)
    O2 = lambda c, j: ("O", c, NBR, j)
    PO = lambda c, j: ("PO", c, j)
    PA = lambda j: ("PH", j, OWN)
    PB = lambda j: ("PH", j, NBR)
    pairs = lambda s, c, g, ps=range(4): [(s, c, g, p) for p in ps]

    def attn(units, fill):
        for n, u in enumerate(units):
            a(("S",) + u)
            for f in fill[n:n + 1] if n + 1 < len(units) else fill[n:]:
                ops.extend(f if isinstance(f, list) else [f])
            a(("P",) + u)

    def chain(units, *fill):
        a(("S",) + units[0])
        for u, v in zip(units, units[1:]):
            a(("S",) + v); a(("P",) + u)
        ops.extend(fill); a(("P",) + units[-1])

    def arrive(*what):
        ops.extend(sorted(what, key=lambda op: op[0] not in ("load", "send")))

    kv = lambda g, c: ("loaded", "kv", g, c)
    wo = lambda j: ("loaded", "wo", j)
    send = lambda *arg: ("send",) + arg
    recv = lambda *arg: ("recv",) + arg
    load = lambda *arg: ("load",) + arg

    for i in range(4):
        a(("load", "wq", i)); a(("load", "x", i))
    a(("flush",))
    a(("first",)); a(("loaded", "x", 0)); a(Q(OWN, 0, OWN, 0))
    arrive(("loaded", "wq", 1)); a(Q(OWN, 0, OWN, 1))
    arrive(("loaded", "x", 1)); a(Q(OWN, 1, OWN, 0)); a(Q(OWN, 1, OWN, 1))
    arrive(("loaded", "wq", 2), load("kv", OWN, 0)); a(Q(OWN, 0, OWN, 2)); a(Q(OWN, 1, OWN, 2))
    arrive(("loaded", "x", 2)); a(Q(OWN, 2, OWN, 0)); a(Q(OWN, 2, OWN, 1))
    arrive(("loaded", "wq", 3), load("kv", OWN, 1)); a(Q(OWN, 2, OWN, 2)); a(Q(OWN, 0, OWN, 3)); a(Q(OWN, 1, OWN, 3))
    arrive(("loaded", "x", 3), load("kv", OWN, 2)); a(Q(OWN, 2, OWN, 3))
    ops.extend(Q(OWN, 3, OWN, p) for p in range(3))
    arrive(recv("wq", 0), load("kv", OWN, 3), load("kv", NBR, 0), load("kv", NBR, 1))
    a(Q(OWN, 3, OWN, 3)); a(Q(OWN, 0, NBR, 0))
    arrive(kv(OWN, 0), recv("x", 0))
    a(Q(OWN, 1, NBR, 0))
    chain(pairs(OWN, 0, OWN, (0, 1)), Q(NBR, 0, OWN, 0))
    chain(pairs(OWN, 0, OWN, (2, 3)), Q(NBR, 0, OWN, 1))
    chain(pairs(NBR, 0, OWN, (0, 1)), kv(OWN, 1), Q(NBR, 0, OWN, 2))
    chain(pairs(OWN, 1, OWN, (0, 1)), Q(NBR, 0, OWN, 3))
    chain(pairs(OWN, 1, OWN, (2, 3)), Q(OWN, 2, NBR, 0))
    chain(pairs(NBR, 0, OWN, (2, 3)), kv(OWN, 2), Q(OWN, 3, NBR, 0))
    chain(pairs(OWN, 2, OWN, (0, 1)), Q(NBR, 0, NBR, 0))
    arrive(recv("wq", 1), load("wo", 0), load("wo", 1), load("kv", NBR, 2), load("kv", NBR, 3), load("wo", 2), load("wo", 3)); a(("flush", 0))
    chain(pairs(OWN, 2, OWN, (2, 3)), Q(OWN, 0, NBR, 1))
    arrive(kv(OWN, 3), recv("x", 1))
    a(Q(OWN, 1, NBR, 1))
    chain(pairs(OWN, 3, OWN, (0, 1)), Q(OWN, 2, NBR, 1))
    chain(pairs(OWN, 3, OWN, (2, 3)), Q(OWN, 3, NBR, 1))
    a(Q(NBR, 1, OWN, 0))
    attn(pairs(NBR, 1, OWN, (0, 1, 2)), [Q(NBR, 1, OWN, 1), Q(NBR, 1, OWN, 2), Q(NBR, 1, OWN, 3)])
    arrive(kv(NBR, 0), kv(NBR, 1))
    a(Q(NBR, 0, NBR, 1))
    attn([(NBR, 1, OWN, 3), (NBR, 0, NBR, 0)], [Q(NBR, 1, NBR, 0), Q(NBR, 1, NBR, 1)])
    arrive(recv("wq", 2)); a(("flush", 0))
    chain([(NBR, 0, NBR, 1)] + pairs(NBR, 1, NBR, (0, 1)), Q(NBR, 0, NBR, 2))
    arrive(recv("x", 2), wo(0), wo(1))
    a(Q(NBR, 1, NBR, 2)); a(Q(NBR, 2, OWN, 0))
    attn(pairs(NBR, 2, OWN), [Q(NBR, 2, OWN, 1), Q(NBR, 2, OWN, 2), Q(NBR, 2, OWN, 3), [O1(0, 0), O1(0, 1)]])
    arrive(kv(NBR, 2), send("wo", 0), send("wo", 1))
    a(Q(NBR, 2, NBR, 0))
    chain([(NBR, 0, NBR, 2), (NBR, 1, NBR, 2)], Q(NBR, 2, NBR, 1))
    chain(pairs(NBR, 2, NBR, (0, 1)), Q(NBR, 2, NBR, 2))
    attn(pairs(NBR, 2, NBR, (2,)), [O1(1, 0)])
    arrive(recv("wq", 3), kv(NBR, 3))
    a(O1(1, 1)); a(Q(NBR, 0, NBR, 3))
    attn([(NBR, 0, NBR, 3)], [Q(NBR, 1, NBR, 3)])
    arrive(recv("x", 3), wo(2), wo(3))
    a(Q(NBR, 2, NBR, 3))
    chain([(NBR, 1, NBR, 3), (NBR, 2, NBR, 3)], Q(NBR, 3, OWN, 0))
    attn(pairs(NBR, 3, OWN), [Q(NBR, 3, OWN, 1), Q(NBR, 3, OWN, 2), Q(NBR, 3, OWN, 3), Q(NBR, 3, NBR, 0)])
    attn(pairs(NBR, 3, NBR, (0, 1)), [Q(NBR, 3, NBR, 1), PA(0)])
    arrive(recv("wo", 0))
    a(PB(0)); a(Q(NBR, 3, NBR, 2)); a(send("wo", 2)); a(PO(1, 0)); a(Q(NBR, 3, NBR, 3))
    attn(pairs(NBR, 3, NBR, (2, 3)), [[send("wo", 3), PO(2, 0)], Q(OWN, 0, NBR, 2)])
    attn(pairs(OWN, 0, NBR), [PO(3, 0), Q(OWN, 0, NBR, 3), Q(OWN, 1, NBR, 2), Q(OWN, 1, NBR, 3)])
    attn(pairs(OWN, 1, NBR, (0, 1)), [Q(OWN, 2, NBR, 2), PA(1)])
    arrive(recv("wo", 1))
    a(PB(1)); a(Q(OWN, 2, NBR, 3)); a(Q(OWN, 3, NBR, 2))
    attn(pairs(OWN, 1, NBR, (2, 3)), [PO(1, 1), PO(2, 1)])
    rest = [O1(c, j) for c, j in ((2, 0), (2, 1), (0, 2), (1, 2), (2, 2), (0, 3), (1, 3), (2, 3), (3, 0), (3, 1), (3, 2), (3, 3))]
    attn(pairs(OWN, 2, NBR), [PO(3, 1), Q(OWN, 3, NBR, 3)] + rest[:2])
    attn(pairs(OWN, 3, NBR, (0, 1, 2)), [rest[2], PA(2)])
    arrive(recv("wo", 2), *(recv("p", c, 0) for c in range(3)))
    a(PB(2)); a(PO(1, 2))
    attn(pairs(OWN, 3, NBR, (3,)), [PO(2, 2)])
    a(PO(3, 2))
    ops.extend(rest[3:])
    for c in range(2):
        a(O2(c, 0)); a(("finish", c, 0))
    a(PA(3))
    arrive(recv("wo", 3), recv("p", 3, 0), *(recv("p", c, 1) for c in range(3)))
    a(PB(3)); a(PO(1, 3)); a(PO(2, 3))
    arrive(recv("p", 3, 1), *(recv("p", c, 2) for c in range(3)))
    a(PO(3, 3))
    for j in range(3):
        for c in range(4):
            if (c, j) == (3, 2):
                arrive(recv("p", 3, 2))
            if j or c >= 2:
                a(O2(c, j)); a(("finish", c, j))
    ops.extend(O2(c, 3) for c in range(3))
    arrive(*(recv("p", c, 3) for c in range(3)))
    ops.extend(("finish", c, 3) for c in range(3))
    a(O2(3, 3))
    arrive(recv("p", 3, 3)); a(("finish", 3, 3))
    return ops


def _lhs_terms(a11, a12, a21, a22):
    return a11 + a22, a21 + a22, a11, a22, a11 + a12, a21 - a11, a12 - a22


def _rhs_terms(b11, b12, b21, b22):
    return b11 + b22, b11, b12 - b22, b21 - b11, b22, b11 + b12, b21 + b22


def _pack2(lo, hi):
    return pltpu.bitcast(pltpu.pack_elementwise([lo, hi], packed_dtype=BF16), U32)


def _half(u, i):
    return pltpu.unpack_elementwise(u, index=i, packed_dtype=BF16, unpacked_dtype=F32)


def _pack(v):
    n, w = v.shape
    v = v.reshape(n // 16, 2, 8, w)
    return _pack2(v[:, 0].reshape(n // 2, w), v[:, 1].reshape(n // 2, w))


def _unpack(u):
    return pltpu.bitcast(u, BF16)


def _body(x_hbm, wq_hbm, k_hbm, v_hbm, wo_hbm, out_ref,
          xf, wqf, wof, kf, vf, xb, wqb, wob, ptx, prx, xs, wqs, wos, cs, qb, acc, half,
          ld_sem, kv_sem, tx_sem, rx_sem):
    me = lax.axis_index("i")
    seq_peer = me ^ 1
    head_peer = 3 - me
    head_shard = (me, head_peer)
    ds = pl.ds

    def remote(src, dst, sem, peer):
        return pltpu.make_async_remote_copy(
            src_ref=src, dst_ref=dst, send_sem=tx_sem.at[sem], recv_sem=rx_sem.at[sem],
            device_id=(peer,), device_id_type=pl.DeviceIdType.MESH)

    cols = lambda j: ds(j * 256, 256)
    load = {
        "x": lambda c: [pltpu.make_async_copy(x_hbm.at[:, c], xf[c], ld_sem.at[c])],
        "wq": lambda p: [pltpu.make_async_copy(wq_hbm.at[:, cols(p)], wqf[p], ld_sem.at[4 + p])] if p else [
            pltpu.make_async_copy(wq_hbm.at[ds(k * 512, 512), cols(0)], wqf[0].at[ds(k * 512, 512)], ld_sem.at[4 + 8 * k])
            for k in range(2)],
        "wo": lambda j: [pltpu.make_async_copy(wo_hbm.at[:, cols(j)], wof[j], ld_sem.at[8 + j])],
        "kv": lambda g, c: [
            pltpu.make_async_copy(src.at[:, c, :, head_shard[g]], dst[g][c], kv_sem.at[(g * 4 + c) * 2 + n])
            for n, (src, dst) in enumerate(((k_hbm, kf), (v_hbm, vf)))],
    }
    swap = {
        "x": lambda c: remote(xb[OWN][c], xb[NBR][c], c, seq_peer),
        "wq": lambda p, rows=ds(0, 512): remote(wqb[OWN][p].at[rows], wqb[NBR][p].at[rows], 4 + p, head_peer),
        "wo": lambda j: remote(wob[OWN][j], wob[NBR][j], 8 + j, head_peer),
        "p": lambda c, j: remote(ptx[c][j], prx[c][j], 12 + c * 4 + j, seq_peer),
    }

    first, queue = [], []
    urgent = lambda tag, *fns: first.extend((tag, fn) for fn in fns)
    later = lambda tag, *fns: queue.extend((tag, fn) for fn in fns)

    def drip(n):
        while first:
            first.pop(0)[1]()
        for _ in range(min(n, len(queue))):
            queue.pop(0)[1]()

    def need(*tags):
        if any(tag in tags for tag, _ in first):
            drip(0)
        for item in [item for item in queue if item[0] in tags]:
            queue.remove(item)
            item[1]()

    def strassen(lhs, rhs, emit, rate):
        def m(i):
            r = jnp.dot(_unpack(lhs(i)), _unpack(rhs(i)), preferred_element_type=F32)
            drip(rate)
            return r
        m1, m3 = m(1), m(3)
        emit(1, 0, m1 + m3)
        m0 = m(0)
        c11, c22 = m0 + m3, m0 - m1
        c11 = c11 + m(6)
        c22 = c22 + m(5)
        m4 = m(4)
        emit(0, 0, c11 - m4)
        m2 = m(2)
        emit(1, 1, c22 + m2)
        emit(0, 1, m2 + m4)

    x_slot, wq_slot = {0: 0, 1: 1, 4: 2, 5: 3, 6: 4}, {0: 0, 2: 1, 3: 2, 5: 3, 6: 4}

    def packed_terms(fn, half):
        lo, hi = (fn(*(half(e, i, k) for i in range(2) for k in range(2))) for e in range(2))
        return lambda i: _pack2(lo[i], hi[i])

    def x_terms(s, c, n):
        if s == OWN:
            half = lambda e, i, k: xf[c][2 * i + n // 4, ds(n % 4 * 16 + e * 8, 8), ds(k * 512, 512)]
        else:
            half = lambda e, i, k: _half(xb[s][c][ds(i * 64 + n * 8, 8), ds(k * 512, 512)], e)
        t = packed_terms(_lhs_terms, half)
        for i, slot in x_slot.items():
            xs[s, c, slot, ds(n * 8, 8), :] = t(i)

    def wq_terms(g, p, n):
        half = lambda e, k, i: _half(wqb[g][p][ds(k * 256 + n * 32, 32), ds(i * 128, 128)], e)
        t = packed_terms(_rhs_terms, half)
        for i, slot in wq_slot.items():
            wqs[g, p, slot, ds(n * 32, 32), :] = t(i)

    def wo_terms(g, j, n):
        row = lambda k: n // 2 * 256 + k * 128 + n % 2 * 64
        half = lambda e, k, i: _half(wob[g][j][ds(row(k) // 2, 32), ds(i * 128, 128)], e)
        t = packed_terms(_rhs_terms, half)
        for i in range(7):
            wos[j, i, ds(g * 256 + n * 32, 32), :] = t(i)

    def x_cast(c, n):
        xb[OWN][c][ds(n * 32, 32), :] = _pack(xf[c][n])

    def wq_cast(p, n):
        v = wqf[p][ds(n * 256, 256), :] * SCALE
        wqb[OWN][p][ds(n * 128, 128), :] = pltpu.bitcast(v.astype(BF16), U32)

    def wo_cast(j, n):
        wob[OWN][j][ds(n * 128, 128), :] = pltpu.bitcast(wof[j][ds(n * 256, 256), :].astype(BF16), U32)

    terms = {"x": x_terms, "wq": wq_terms, "wo": wo_terms}
    cast = {"x": x_cast, "wq": wq_cast, "wo": wo_cast}

    def x_term(s, c, i):
        if i in x_slot:
            return xs[s, c, x_slot[i]]
        return xb[s][c][ds(0, 64), ds(0, 512)] if i == 2 else xb[s][c][ds(64, 64), ds(512, 512)]

    def wq_term(g, p, i):
        if i in wq_slot:
            return wqs[g, p, wq_slot[i]]
        return wqb[g][p][ds(0, 256), ds(0, 128)] if i == 1 else wqb[g][p][ds(256, 256), ds(128, 128)]

    def head(ref, g, c, h):
        return ref[g][c].reshape(2048, 128)[ds(h, 256, stride=8), :].astype(BF16)

    def finish(c, j, m):
        mine = acc[c, j, ds(m * 64, 64), :].reshape(4, 2, 8, 256)
        theirs = prx[c][j][ds(m * 32, 32), :]
        r = _pack2(*(mine[:, e].reshape(32, 256) + _half(theirs, e) for e in range(2)))
        out_ref[0, ds((4 * m + c) * 64, 64), cols(j)] = _unpack(r)

    barrier = pltpu.get_barrier_semaphore()
    for peer in (seq_peer, head_peer):
        pl.semaphore_signal(barrier, inc=1, device_id=(peer,), device_id_type=pl.DeviceIdType.MESH)

    probs, sent = {}, []

    def send(name, *idx):
        swap[name](*idx).start()
        sent.append((name, *idx))

    def run(op, *arg):
        if op == "load":
            urgent(None, lambda: [d.start() for d in load[arg[0]](*arg[1:])])
        elif op == "first":
            for k, d in enumerate(load["wq"](0)):
                d.wait()
                wq_cast(0, 2 * k); wq_cast(0, 2 * k + 1)
                if k == 0:
                    pl.semaphore_wait(barrier, 2)
                swap["wq"](0, ds(k * 256, 256)).start()
            sent.append(("wq", 0))
            for k in range(8):
                wq_terms(OWN, 0, k)
        elif op == "loaded":
            name, *idx = arg
            tag = (name, *idx) if name == "kv" else (name, OWN, *idx)
            urgent(tag, lambda: [d.wait() for d in load[name](*idx)])
            if name != "kv":
                later(tag, *(partial(cast[name], *idx, k) for k in range(4)))
                if name != "wo":
                    later(tag, partial(send, name, *idx))
                later(tag, *(partial(terms[name], OWN, *idx, k) for k in range(8)))
        elif op == "send":
            name, *idx = arg
            need((name, OWN, *idx))
            urgent(None, partial(send, name, *idx))
        elif op == "recv":
            name, *idx = arg
            tag = (name, NBR, *idx)
            urgent(tag, lambda: swap[name](*idx).wait_recv())
            if name != "p":
                later(tag, *(partial(terms[name], NBR, *idx, k) for k in range(8)))
        elif op == "flush":
            drip(*(arg or [len(queue)]))
        elif op == "Q":
            s, c, g, p = arg
            need(("x", s, c), ("wq", g, p))

            def emit(i, k, v):
                qb[s, c, g, ds(i * 64, 64), ds(p * 256 + k * 128, 128)] = _pack(v)
            strassen(lambda i: x_term(s, c, i), lambda i: wq_term(g, p, i), emit, 1)
        elif op == "S":
            s, c, g, p = arg
            need(("kv", g, c))
            for h in (2 * p, 2 * p + 1):
                q = _unpack(qb[s, c, g, :, ds(h * 128, 128)])
                sc = lax.dot_general(q, head(kf, g, c, h), (((1,), (1,)), ((), ())), preferred_element_type=F32)
                e = jnp.exp2(sc - jnp.max(sc, axis=1, keepdims=True))
                total = jnp.sum(e, axis=1, keepdims=True)
                r = pl.reciprocal(total, approx=True)
                probs[s, c, g, h] = (e.astype(BF16), r * (2.0 - total * r))
        elif op == "P":
            s, c, g, p = arg
            o = []
            for h in (2 * p, 2 * p + 1):
                e, r = probs.pop((s, c, g, h))
                o.append(jnp.dot(e, head(vf, g, c, h), preferred_element_type=F32) * r)
            for i, t in enumerate(_lhs_terms(o[0][:128], o[1][:128], o[0][128:], o[1][128:])):
                cs[s, c, i, :, ds(g * 512 + p * 128, 128)] = _pack(t)
        elif op == "O":
            c, g, j = arg
            need(("wo", g, j))

            def emit(i, k, v):
                at = (c, j, ds(i * 128, 128), ds(k * 128, 128))
                acc[at] = v if g == OWN else acc[at] + v
            strassen(lambda i: cs[OWN, c, i, :, ds(g * 512, 512)], lambda i: wos[j, i, ds(g * 256, 256), :], emit, 1)
        elif op == "PO":
            c, j = arg
            need(("wo", OWN, j), ("wo", NBR, j))

            def emit(i, k, v):
                ptx[c][j][ds(i * 64, 64), ds(k * 128, 128)] = _pack(v)
            strassen(lambda i: cs[NBR, c, i], lambda i: wos[j, i], emit, 2)
            urgent(None, partial(send, "p", c, j))
        elif op == "PH":
            j, g = arg
            need(("wo", g, j))

            def emit(i, k, v):
                at = (j, ds(i * 128, 128), ds(k * 128, 128))
                if g == OWN:
                    half[at] = v
                else:
                    ptx[0][j][ds(i * 64, 64), ds(k * 128, 128)] = _pack(half[at] + v)
            strassen(lambda i: cs[NBR, 0, i, :, ds(g * 512, 512)], lambda i: wos[j, i, ds(g * 256, 256), :], emit, 1)
            if g == NBR:
                urgent(None, partial(send, "p", 0, j))
        elif op == "finish":
            later(None, *(partial(finish, *arg, m) for m in range(4)))
        else:
            raise ValueError(op)

    for step in _schedule():
        run(*step)
    drip(len(queue))
    for name, *idx in sent:
        swap[name](*idx).wait_send()


def pallas_dist_sparse_attn_strided_qseq_b1_sq1024_skv1024_hq8_dh128_kernel(x, Wq, K_ext, V_ext, Wo):
    def bufs(count, shape, dtype):
        if not count:
            return pltpu.VMEM(shape, dtype)
        return [bufs(count[1:], shape, dtype) for _ in range(count[0])]

    hbm = pl.BlockSpec(memory_space=pltpu.MemorySpace.HBM)
    return pl.pallas_call(
        _body,
        out_shape=jax.ShapeDtypeStruct((1, 1024, 1024), BF16),
        in_specs=[hbm] * 5,
        out_specs=pl.BlockSpec(memory_space=pltpu.MemorySpace.VMEM),
        scratch_shapes=[
            bufs((4,), (4, 64, 1024), F32),
            bufs((4,), (1024, 256), F32),
            bufs((4,), (1024, 256), F32),
            bufs((2, 4), (4, 64, 8, 128), F32),
            bufs((2, 4), (4, 64, 8, 128), F32),
            bufs((2, 4), (128, 1024), U32),
            bufs((2, 4), (512, 256), U32),
            bufs((2, 4), (512, 256), U32),
            bufs((4, 4), (128, 256), U32),
            bufs((4, 4), (128, 256), U32),
            pltpu.VMEM((2, 4, 5, 64, 512), U32),
            pltpu.VMEM((2, 4, 5, 256, 128), U32),
            pltpu.VMEM((4, 7, 512, 128), U32),
            pltpu.VMEM((2, 4, 7, 64, 1024), U32),
            pltpu.VMEM((2, 4, 2, 128, 1024), U32),
            pltpu.VMEM((4, 4, 256, 256), F32),
            pltpu.VMEM((4, 256, 256), F32),
            pltpu.SemaphoreType.DMA((13,)),
            pltpu.SemaphoreType.DMA((16,)),
            pltpu.SemaphoreType.DMA((28,)),
            pltpu.SemaphoreType.DMA((28,)),
        ],
        compiler_params=pltpu.CompilerParams(collective_id=0, vmem_limit_bytes=110 * 1024 * 1024),
    )(x.reshape(4, 4, 64, 1024), Wq, K_ext.reshape(4, 4, 64, 4, 8, 128), V_ext.reshape(4, 4, 64, 4, 8, 128), Wo)
```

```python
from functools import partial
import jax
import jax.numpy as jnp
from jax import lax
from jax.experimental import pallas as pl
from jax.experimental.pallas import tpu as pltpu

F32, BF16, U32 = jnp.float32, jnp.bfloat16, jnp.uint32
SCALE = 0.08838834764831843 * 1.4426950408889634
OWN, NBR = 0, 1


def _schedule():
    ops = []
    a = ops.append
    Q = lambda s, c, g, p: ("Q", s, c, g, p)
    O1 = lambda c, j: ("O", c, OWN, j)
    O2 = lambda c, j: ("O", c, NBR, j)
    PO = lambda c, j: ("PO", c, j)
    PA = lambda j: ("PH", j, OWN)
    PB = lambda j: ("PH", j, NBR)
    pairs = lambda s, c, g, ps=range(4): [(s, c, g, p) for p in ps]

    def attn(units, fill):
        for n, u in enumerate(units):
            a(("S",) + u)
            for f in fill[n:n + 1] if n + 1 < len(units) else fill[n:]:
                ops.extend(f if isinstance(f, list) else [f])
            a(("P",) + u)

    def chain(units, *fill):
        a(("S",) + units[0])
        for u, v in zip(units, units[1:]):
            a(("S",) + v); a(("P",) + u)
        ops.extend(fill); a(("P",) + units[-1])

    def arrive(*what):
        ops.extend(sorted(what, key=lambda op: op[0] not in ("load", "send")))

    kv = lambda g, c: ("loaded", "kv", g, c)
    wo = lambda j: ("loaded", "wo", j)
    send = lambda *arg: ("send",) + arg
    recv = lambda *arg: ("recv",) + arg
    load = lambda *arg: ("load",) + arg

    for i in range(4):
        a(("load", "wq", i)); a(("load", "x", i))
    ops.extend(load("kv", OWN, c) for c in range(3))
    a(("flush",))
    a(("first",)); a(("loaded", "x", 0)); a(Q(OWN, 0, OWN, 0))
    arrive(("loaded", "wq", 1)); a(Q(OWN, 0, OWN, 1))
    arrive(("loaded", "x", 1)); a(Q(OWN, 1, OWN, 0)); a(Q(OWN, 1, OWN, 1))
    arrive(("loaded", "wq", 2)); a(Q(OWN, 0, OWN, 2)); a(Q(OWN, 1, OWN, 2))
    arrive(("loaded", "x", 2)); a(Q(OWN, 2, OWN, 0)); a(Q(OWN, 2, OWN, 1))
    arrive(("loaded", "wq", 3)); a(Q(OWN, 2, OWN, 2)); a(Q(OWN, 0, OWN, 3)); a(Q(OWN, 1, OWN, 3))
    arrive(("loaded", "x", 3)); a(Q(OWN, 2, OWN, 3))
    ops.extend(Q(OWN, 3, OWN, p) for p in range(3))
    arrive(recv("wq", 0), load("kv", OWN, 3), load("kv", NBR, 0), load("kv", NBR, 1))
    a(Q(OWN, 3, OWN, 3)); a(Q(OWN, 0, NBR, 0))
    arrive(kv(OWN, 0), recv("x", 0))
    a(Q(OWN, 1, NBR, 0))
    chain(pairs(OWN, 0, OWN, (0, 1)), Q(NBR, 0, OWN, 0))
    chain(pairs(OWN, 0, OWN, (2, 3)), Q(NBR, 0, OWN, 1))
    chain(pairs(NBR, 0, OWN, (0, 1)), kv(OWN, 1), Q(NBR, 0, OWN, 2))
    chain(pairs(OWN, 1, OWN, (0, 1)), Q(NBR, 0, OWN, 3))
    chain(pairs(OWN, 1, OWN, (2, 3)), Q(OWN, 2, NBR, 0))
    chain(pairs(NBR, 0, OWN, (2, 3)), kv(OWN, 2), Q(OWN, 3, NBR, 0))
    chain(pairs(OWN, 2, OWN, (0, 1)), Q(NBR, 0, NBR, 0))
    arrive(recv("wq", 1), load("wo", 0), load("wo", 1), load("kv", NBR, 2), load("kv", NBR, 3), load("wo", 2), load("wo", 3)); a(("flush", 0))
    chain(pairs(OWN, 2, OWN, (2, 3)), Q(OWN, 0, NBR, 1))
    arrive(kv(OWN, 3), recv("x", 1))
    a(Q(OWN, 1, NBR, 1))
    chain(pairs(OWN, 3, OWN, (0, 1)), Q(OWN, 2, NBR, 1))
    chain(pairs(OWN, 3, OWN, (2, 3)), Q(OWN, 3, NBR, 1))
    a(Q(NBR, 1, OWN, 0))
    attn(pairs(NBR, 1, OWN, (0, 1, 2)), [Q(NBR, 1, OWN, 1), Q(NBR, 1, OWN, 2), Q(NBR, 1, OWN, 3)])
    arrive(kv(NBR, 0), kv(NBR, 1))
    a(Q(NBR, 0, NBR, 1))
    attn([(NBR, 1, OWN, 3), (NBR, 0, NBR, 0)], [Q(NBR, 1, NBR, 0), Q(NBR, 1, NBR, 1)])
    arrive(recv("wq", 2)); a(("flush", 0))
    chain([(NBR, 0, NBR, 1)] + pairs(NBR, 1, NBR, (0, 1)), Q(NBR, 0, NBR, 2))
    arrive(recv("x", 2), wo(0), wo(1))
    a(Q(NBR, 1, NBR, 2)); a(Q(NBR, 2, OWN, 0))
    attn(pairs(NBR, 2, OWN), [Q(NBR, 2, OWN, 1), Q(NBR, 2, OWN, 2), Q(NBR, 2, OWN, 3), [O1(0, 0), O1(0, 1)]])
    arrive(kv(NBR, 2), send("wo", 0), send("wo", 1))
    a(Q(NBR, 2, NBR, 0))
    chain([(NBR, 0, NBR, 2), (NBR, 1, NBR, 2)], Q(NBR, 2, NBR, 1))
    chain(pairs(NBR, 2, NBR, (0, 1)), Q(NBR, 2, NBR, 2))
    attn(pairs(NBR, 2, NBR, (2,)), [O1(1, 0)])
    arrive(recv("wq", 3), kv(NBR, 3))
    a(O1(1, 1)); a(Q(NBR, 0, NBR, 3))
    attn([(NBR, 0, NBR, 3)], [Q(NBR, 1, NBR, 3)])
    arrive(recv("x", 3), wo(2), wo(3))
    a(Q(NBR, 2, NBR, 3))
    chain([(NBR, 1, NBR, 3), (NBR, 2, NBR, 3)], Q(NBR, 3, OWN, 0))
    attn(pairs(NBR, 3, OWN), [Q(NBR, 3, OWN, 1), Q(NBR, 3, OWN, 2), Q(NBR, 3, OWN, 3), Q(NBR, 3, NBR, 0)])
    attn(pairs(NBR, 3, NBR, (0, 1)), [Q(NBR, 3, NBR, 1), PA(0)])
    arrive(recv("wo", 0))
    a(PB(0)); a(Q(NBR, 3, NBR, 2)); a(send("wo", 2)); a(PO(1, 0)); a(Q(NBR, 3, NBR, 3))
    attn(pairs(NBR, 3, NBR, (2, 3)), [[send("wo", 3), PO(2, 0)], Q(OWN, 0, NBR, 2)])
    attn(pairs(OWN, 0, NBR), [PO(3, 0), Q(OWN, 0, NBR, 3), Q(OWN, 1, NBR, 2), Q(OWN, 1, NBR, 3)])
    attn(pairs(OWN, 1, NBR, (0, 1)), [Q(OWN, 2, NBR, 2), PA(1)])
    arrive(recv("wo", 1))
    a(PB(1)); a(Q(OWN, 2, NBR, 3)); a(Q(OWN, 3, NBR, 2))
    attn(pairs(OWN, 1, NBR, (2, 3)), [PO(1, 1), PO(2, 1)])
    rest = [O1(c, j) for c, j in ((2, 0), (2, 1), (0, 2), (1, 2), (2, 2), (0, 3), (1, 3), (2, 3), (3, 0), (3, 1), (3, 2), (3, 3))]
    attn(pairs(OWN, 2, NBR), [PO(3, 1), Q(OWN, 3, NBR, 3)] + rest[:2])
    attn(pairs(OWN, 3, NBR, (0, 1, 2)), [rest[2], PA(2)])
    arrive(recv("wo", 2), *(recv("p", c, 0) for c in range(3)))
    a(PB(2)); a(PO(1, 2))
    attn(pairs(OWN, 3, NBR, (3,)), [PO(2, 2)])
    a(PO(3, 2))
    ops.extend(rest[3:])
    for c in range(2):
        a(O2(c, 0)); a(("finish", c, 0))
    a(PA(3))
    arrive(recv("wo", 3), recv("p", 3, 0), *(recv("p", c, 1) for c in range(3)))
    a(PB(3)); a(PO(1, 3)); a(PO(2, 3))
    arrive(recv("p", 3, 1), *(recv("p", c, 2) for c in range(3)))
    a(PO(3, 3))
    for j in range(3):
        for c in range(4):
            if (c, j) == (3, 2):
                arrive(recv("p", 3, 2))
            if j or c >= 2:
                a(O2(c, j)); a(("finish", c, j))
    ops.extend(O2(c, 3) for c in range(3))
    arrive(*(recv("p", c, 3) for c in range(3)))
    ops.extend(("finish", c, 3) for c in range(3))
    a(O2(3, 3))
    arrive(recv("p", 3, 3)); a(("finish", 3, 3))
    return ops


def _lhs_terms(a11, a12, a21, a22):
    return a11 + a22, a21 + a22, a11, a22, a11 + a12, a21 - a11, a12 - a22


def _rhs_terms(b11, b12, b21, b22):
    return b11 + b22, b11, b12 - b22, b21 - b11, b22, b11 + b12, b21 + b22


def _pack2(lo, hi):
    return pltpu.bitcast(pltpu.pack_elementwise([lo, hi], packed_dtype=BF16), U32)


def _half(u, i):
    return pltpu.unpack_elementwise(u, index=i, packed_dtype=BF16, unpacked_dtype=F32)


def _pack(v):
    n, w = v.shape
    v = v.reshape(n // 16, 2, 8, w)
    return _pack2(v[:, 0].reshape(n // 2, w), v[:, 1].reshape(n // 2, w))


def _unpack(u):
    return pltpu.bitcast(u, BF16)


def _body(x_hbm, wq_hbm, k_hbm, v_hbm, wo_hbm, out_ref,
          xf, wqf, wof, kf, vf, xb, wqb, wob, ptx, prx, xs, wqs, wos, cs, qb, acc, half,
          ld_sem, kv_sem, tx_sem, rx_sem):
    me = lax.axis_index("i")
    seq_peer = me ^ 1
    head_peer = 3 - me
    head_shard = (me, head_peer)
    ds = pl.ds

    def remote(src, dst, sem, peer):
        return pltpu.make_async_remote_copy(
            src_ref=src, dst_ref=dst, send_sem=tx_sem.at[sem], recv_sem=rx_sem.at[sem],
            device_id=(peer,), device_id_type=pl.DeviceIdType.MESH)

    cols = lambda j: ds(j * 256, 256)
    load = {
        "x": lambda c: [pltpu.make_async_copy(x_hbm.at[:, c], xf[c], ld_sem.at[c])],
        "wq": lambda p: [pltpu.make_async_copy(wq_hbm.at[:, cols(p)], wqf[p], ld_sem.at[4 + p])] if p else [
            pltpu.make_async_copy(wq_hbm.at[ds(k * 512, 512), cols(0)], wqf[0].at[ds(k * 512, 512)], ld_sem.at[4 + 8 * k])
            for k in range(2)],
        "wo": lambda j: [pltpu.make_async_copy(wo_hbm.at[:, cols(j)], wof[j], ld_sem.at[8 + j])],
        "kv": lambda g, c: [
            pltpu.make_async_copy(src.at[:, c, :, head_shard[g]], dst[g][c], kv_sem.at[(g * 4 + c) * 2 + n])
            for n, (src, dst) in enumerate(((k_hbm, kf), (v_hbm, vf)))],
    }
    swap = {
        "x": lambda c: remote(xb[OWN][c], xb[NBR][c], c, seq_peer),
        "wq": lambda p, rows=ds(0, 512): remote(wqb[OWN][p].at[rows], wqb[NBR][p].at[rows], 4 + p, head_peer),
        "wo": lambda j: remote(wob[OWN][j], wob[NBR][j], 8 + j, head_peer),
        "p": lambda c, j: remote(ptx[c][j], prx[c][j], 12 + c * 4 + j, seq_peer),
    }

    first, queue = [], []
    urgent = lambda tag, *fns: first.extend((tag, fn) for fn in fns)
    later = lambda tag, *fns: queue.extend((tag, fn) for fn in fns)

    def drip(n):
        while first:
            first.pop(0)[1]()
        for _ in range(min(n, len(queue))):
            queue.pop(0)[1]()

    def need(*tags):
        if any(tag in tags for tag, _ in first):
            drip(0)
        for item in [item for item in queue if item[0] in tags]:
            queue.remove(item)
            item[1]()

    def strassen(lhs, rhs, emit, rate):
        def m(i):
            r = jnp.dot(_unpack(lhs(i)), _unpack(rhs(i)), preferred_element_type=F32)
            drip(rate)
            return r
        m1, m3 = m(1), m(3)
        emit(1, 0, m1 + m3)
        m0 = m(0)
        c11, c22 = m0 + m3, m0 - m1
        c11 = c11 + m(6)
        c22 = c22 + m(5)
        m4 = m(4)
        emit(0, 0, c11 - m4)
        m2 = m(2)
        emit(1, 1, c22 + m2)
        emit(0, 1, m2 + m4)

    x_slot, wq_slot = {0: 0, 1: 1, 4: 2, 5: 3, 6: 4}, {0: 0, 2: 1, 3: 2, 5: 3, 6: 4}

    def packed_terms(fn, half):
        lo, hi = (fn(*(half(e, i, k) for i in range(2) for k in range(2))) for e in range(2))
        return lambda i: _pack2(lo[i], hi[i])

    def x_terms(s, c, n):
        if s == OWN:
            half = lambda e, i, k: xf[c][2 * i + n // 4, ds(n % 4 * 16 + e * 8, 8), ds(k * 512, 512)]
        else:
            half = lambda e, i, k: _half(xb[s][c][ds(i * 64 + n * 8, 8), ds(k * 512, 512)], e)
        t = packed_terms(_lhs_terms, half)
        for i, slot in x_slot.items():
            xs[s, c, slot, ds(n * 8, 8), :] = t(i)

    def wq_terms(g, p, n):
        half = lambda e, k, i: _half(wqb[g][p][ds(k * 256 + n * 32, 32), ds(i * 128, 128)], e)
        t = packed_terms(_rhs_terms, half)
        for i, slot in wq_slot.items():
            wqs[g, p, slot, ds(n * 32, 32), :] = t(i)

    def wo_terms(g, j, n):
        row = lambda k: n // 2 * 256 + k * 128 + n % 2 * 64
        half = lambda e, k, i: _half(wob[g][j][ds(row(k) // 2, 32), ds(i * 128, 128)], e)
        t = packed_terms(_rhs_terms, half)
        for i in range(7):
            wos[j, i, ds(g * 256 + n * 32, 32), :] = t(i)

    def x_cast(c, n):
        xb[OWN][c][ds(n * 32, 32), :] = _pack(xf[c][n])

    def wq_cast(p, n):
        v = wqf[p][ds(n * 256, 256), :] * SCALE
        wqb[OWN][p][ds(n * 128, 128), :] = pltpu.bitcast(v.astype(BF16), U32)

    def wo_cast(j, n):
        wob[OWN][j][ds(n * 128, 128), :] = pltpu.bitcast(wof[j][ds(n * 256, 256), :].astype(BF16), U32)

    terms = {"x": x_terms, "wq": wq_terms, "wo": wo_terms}
    cast = {"x": x_cast, "wq": wq_cast, "wo": wo_cast}

    def x_term(s, c, i):
        if i in x_slot:
            return xs[s, c, x_slot[i]]
        return xb[s][c][ds(0, 64), ds(0, 512)] if i == 2 else xb[s][c][ds(64, 64), ds(512, 512)]

    def wq_term(g, p, i):
        if i in wq_slot:
            return wqs[g, p, wq_slot[i]]
        return wqb[g][p][ds(0, 256), ds(0, 128)] if i == 1 else wqb[g][p][ds(256, 256), ds(128, 128)]

    def head(ref, g, c, h):
        return ref[g][c].reshape(2048, 128)[ds(h, 256, stride=8), :].astype(BF16)

    def finish(c, j, m):
        mine = acc[c, j, ds(m * 64, 64), :].reshape(4, 2, 8, 256)
        theirs = prx[c][j][ds(m * 32, 32), :]
        r = _pack2(*(mine[:, e].reshape(32, 256) + _half(theirs, e) for e in range(2)))
        out_ref[0, ds((4 * m + c) * 64, 64), cols(j)] = _unpack(r)

    barrier = pltpu.get_barrier_semaphore()
    for peer in (seq_peer, head_peer):
        pl.semaphore_signal(barrier, inc=1, device_id=(peer,), device_id_type=pl.DeviceIdType.MESH)

    probs, sent = {}, []

    def send(name, *idx):
        swap[name](*idx).start()
        sent.append((name, *idx))

    def run(op, *arg):
        if op == "load":
            urgent(None, lambda: [d.start() for d in load[arg[0]](*arg[1:])])
        elif op == "first":
            for k, d in enumerate(load["wq"](0)):
                d.wait()
                wq_cast(0, 2 * k); wq_cast(0, 2 * k + 1)
                if k == 0:
                    pl.semaphore_wait(barrier, 2)
                swap["wq"](0, ds(k * 256, 256)).start()
            sent.append(("wq", 0))
            for k in range(8):
                wq_terms(OWN, 0, k)
        elif op == "loaded":
            name, *idx = arg
            tag = (name, *idx) if name == "kv" else (name, OWN, *idx)
            urgent(tag, lambda: [d.wait() for d in load[name](*idx)])
            if name != "kv":
                later(tag, *(partial(cast[name], *idx, k) for k in range(4)))
                if name != "wo":
                    later(tag, partial(send, name, *idx))
                later(tag, *(partial(terms[name], OWN, *idx, k) for k in range(8)))
        elif op == "send":
            name, *idx = arg
            need((name, OWN, *idx))
            urgent(None, partial(send, name, *idx))
        elif op == "recv":
            name, *idx = arg
            tag = (name, NBR, *idx)
            urgent(tag, lambda: swap[name](*idx).wait_recv())
            if name != "p":
                later(tag, *(partial(terms[name], NBR, *idx, k) for k in range(8)))
        elif op == "flush":
            drip(*(arg or [len(queue)]))
        elif op == "Q":
            s, c, g, p = arg
            need(("x", s, c), ("wq", g, p))

            def emit(i, k, v):
                qb[s, c, g, ds(i * 64, 64), ds(p * 256 + k * 128, 128)] = _pack(v)
            strassen(lambda i: x_term(s, c, i), lambda i: wq_term(g, p, i), emit, 1)
        elif op == "S":
            s, c, g, p = arg
            need(("kv", g, c))
            for h in (2 * p, 2 * p + 1):
                q = _unpack(qb[s, c, g, :, ds(h * 128, 128)])
                sc = lax.dot_general(q, head(kf, g, c, h), (((1,), (1,)), ((), ())), preferred_element_type=F32)
                e = jnp.exp2(sc - jnp.max(sc, axis=1, keepdims=True))
                total = jnp.sum(e, axis=1, keepdims=True)
                r = pl.reciprocal(total, approx=True)
                probs[s, c, g, h] = (e.astype(BF16), r * (2.0 - total * r))
        elif op == "P":
            s, c, g, p = arg
            o = []
            for h in (2 * p, 2 * p + 1):
                e, r = probs.pop((s, c, g, h))
                o.append(jnp.dot(e, head(vf, g, c, h), preferred_element_type=F32) * r)
            for i, t in enumerate(_lhs_terms(o[0][:128], o[1][:128], o[0][128:], o[1][128:])):
                cs[s, c, i, :, ds(g * 512 + p * 128, 128)] = _pack(t)
        elif op == "O":
            c, g, j = arg
            need(("wo", g, j))

            def emit(i, k, v):
                at = (c, j, ds(i * 128, 128), ds(k * 128, 128))
                acc[at] = v if g == OWN else acc[at] + v
            strassen(lambda i: cs[OWN, c, i, :, ds(g * 512, 512)], lambda i: wos[j, i, ds(g * 256, 256), :], emit, 1)
        elif op == "PO":
            c, j = arg
            need(("wo", OWN, j), ("wo", NBR, j))

            def emit(i, k, v):
                ptx[c][j][ds(i * 64, 64), ds(k * 128, 128)] = _pack(v)
            strassen(lambda i: cs[NBR, c, i], lambda i: wos[j, i], emit, 2)
            urgent(None, partial(send, "p", c, j))
        elif op == "PH":
            j, g = arg
            need(("wo", g, j))

            def emit(i, k, v):
                at = (j, ds(i * 128, 128), ds(k * 128, 128))
                if g == OWN:
                    half[at] = v
                else:
                    ptx[0][j][ds(i * 64, 64), ds(k * 128, 128)] = _pack(half[at] + v)
            strassen(lambda i: cs[NBR, 0, i, :, ds(g * 512, 512)], lambda i: wos[j, i, ds(g * 256, 256), :], emit, 1)
            if g == NBR:
                urgent(None, partial(send, "p", 0, j))
        elif op == "finish":
            later(None, *(partial(finish, *arg, m) for m in range(4)))
        else:
            raise ValueError(op)

    for step in _schedule():
        run(*step)
    drip(len(queue))
    for name, *idx in sent:
        swap[name](*idx).wait_send()


def pallas_dist_sparse_attn_strided_qseq_b1_sq1024_skv1024_hq8_dh128_kernel(x, Wq, K_ext, V_ext, Wo):
    def bufs(count, shape, dtype):
        if not count:
            return pltpu.VMEM(shape, dtype)
        return [bufs(count[1:], shape, dtype) for _ in range(count[0])]

    hbm = pl.BlockSpec(memory_space=pltpu.MemorySpace.HBM)
    return pl.pallas_call(
        _body,
        out_shape=jax.ShapeDtypeStruct((1, 1024, 1024), BF16),
        in_specs=[hbm] * 5,
        out_specs=pl.BlockSpec(memory_space=pltpu.MemorySpace.VMEM),
        scratch_shapes=[
            bufs((4,), (4, 64, 1024), F32),
            bufs((4,), (1024, 256), F32),
            bufs((4,), (1024, 256), F32),
            bufs((2, 4), (4, 64, 8, 128), F32),
            bufs((2, 4), (4, 64, 8, 128), F32),
            bufs((2, 4), (128, 1024), U32),
            bufs((2, 4), (512, 256), U32),
            bufs((2, 4), (512, 256), U32),
            bufs((4, 4), (128, 256), U32),
            bufs((4, 4), (128, 256), U32),
            pltpu.VMEM((2, 4, 5, 64, 512), U32),
            pltpu.VMEM((2, 4, 5, 256, 128), U32),
            pltpu.VMEM((4, 7, 512, 128), U32),
            pltpu.VMEM((2, 4, 7, 64, 1024), U32),
            pltpu.VMEM((2, 4, 2, 128, 1024), U32),
            pltpu.VMEM((4, 4, 256, 256), F32),
            pltpu.VMEM((4, 256, 256), F32),
            pltpu.SemaphoreType.DMA((13,)),
            pltpu.SemaphoreType.DMA((16,)),
            pltpu.SemaphoreType.DMA((28,)),
            pltpu.SemaphoreType.DMA((28,)),
        ],
        compiler_params=pltpu.CompilerParams(collective_id=0, vmem_limit_bytes=110 * 1024 * 1024),
    )(x.reshape(4, 4, 64, 1024), Wq, K_ext.reshape(4, 4, 64, 4, 8, 128), V_ext.reshape(4, 4, 64, 4, 8, 128), Wo)
```
